```python
import numpy as np

kernel_name = "dist_ring_attn_i_s256_d64"

def setup_inputs():
    S, D = 1024, 64
    q = np.random.randn(S, D).astype(np.float32)
    k = np.random.randn(S, D).astype(np.float32)
    v = np.random.randn(S, D).astype(np.float32)
    return {"q": q, "k": k, "v": v}

def reference(q: np.ndarray, k: np.ndarray, v: np.ndarray) -> np.ndarray:
    D = q.shape[1]
    scores = q @ k.T / np.sqrt(D)
    scores_max = np.max(scores, axis=1, keepdims=True)
    weights = np.exp(scores - scores_max)
    weights = weights / np.sum(weights, axis=1, keepdims=True)
    return weights @ v
```

```python
import jax
import jax.numpy as jnp
from jax import lax
from jax.experimental import pallas as pl
from jax.experimental.pallas import tpu as pltpu

_N_DEV = 4
_MESH = pl.DeviceIdType.MESH
_BF16 = jnp.bfloat16
_F32 = jnp.float32
_U32 = jnp.uint32
_NT = (((1,), (1,)), ((), ()))
_LOG2E = 1.4426950408889634

_N_RELAY = 8
_K_FIRST = 16


def pallas_dist_ring_attn_i_s256_d64_kernel(
    q: jax.Array,
    k: jax.Array,
    v: jax.Array,
):
    S, D = q.shape
    H = S // 2
    W = D // 2
    HB = 2 * W
    RB = HB // _N_RELAY
    scale = _LOG2E / (D**0.5)

    def body(
        qt_hbm, kt_hbm, vt_hbm, out_ref,
        q32, k32, v32, kv, q16, p16,
        load_sems, send_sems, recv_sems, ready_sem,
    ):
        me = lax.axis_index("i")
        right = (me + 1) % _N_DEV
        left = (me + _N_DEV - 1) % _N_DEV

        first_right = me >= 2
        first_left = (me == 1) | (me == 2)
        later_right = jnp.logical_not(first_right)
        later_left = jnp.logical_not(first_left)

        def signal(sem, target):
            pl.semaphore_signal(sem, inc=1, device_id=(target,), device_id_type=_MESH)

        barrier = pltpu.get_barrier_semaphore()
        pl.when(later_right)(lambda: signal(barrier, right))
        pl.when(later_left)(lambda: signal(barrier, left))

        load_k0 = pltpu.make_async_copy(
            kt_hbm.at[pl.ds(0, _K_FIRST)], k32.at[pl.ds(0, _K_FIRST)], load_sems.at[0]
        )
        load_k1 = pltpu.make_async_copy(
            kt_hbm.at[pl.ds(_K_FIRST, D - _K_FIRST)],
            k32.at[pl.ds(_K_FIRST, D - _K_FIRST)],
            load_sems.at[1],
        )
        load_v = pltpu.make_async_copy(vt_hbm, v32, load_sems.at[2])
        load_q = pltpu.make_async_copy(qt_hbm, q32, load_sems.at[3])
        load_k0.start()
        load_k1.start()
        load_v.start()
        load_q.start()

        pl.when(me == 2)(lambda: pl.semaphore_wait(barrier, 2))
        pl.when((me == 1) | (me == 3))(lambda: pl.semaphore_wait(barrier, 1))
        pl.when(first_left)(lambda: signal(ready_sem, left))
        pl.when(first_right)(lambda: signal(ready_sem, right))

        def rows(slot, start, size):
            return kv.at[slot, pl.ds(start, size)]

        n_send = [0]

        def remote(src, dst, target, recv_sem):
            i = n_send[0]
            n_send[0] += 1
            return pltpu.make_async_remote_copy(
                src_ref=src,
                dst_ref=dst,
                send_sem=send_sems.at[i],
                recv_sem=recv_sems.at[recv_sem],
                device_id=(target,),
                device_id_type=_MESH,
            )

        R = _N_RELAY
        SEM_L, SEM_R, SEM_L_REST, SEM_R_REST, SEM_DK, SEM_DV = (
            0, R, 2 * R, 2 * R + 1, 2 * R + 2, 2 * R + 3,
        )
        to_right = [
            remote(rows(0, j * RB, RB), rows(1, j * RB, RB), right, SEM_L + j)
            for j in range(R)
        ] + [remote(rows(0, HB, HB), rows(1, HB, HB), right, SEM_L_REST)]
        to_left = [
            remote(rows(0, HB + j * RB, RB), rows(2, HB + j * RB, RB), left, SEM_R + j)
            for j in range(R)
        ] + [remote(rows(0, 0, HB), rows(2, 0, HB), left, SEM_R_REST)]

        def start_first(lo, hi):
            @pl.when(first_right)
            def _():
                for c in to_right[lo:hi]:
                    c.start()

            @pl.when(first_left)
            def _():
                for c in to_left[lo:hi]:
                    c.start()

        def round_to_bf16(src, row, n, dst_a, dst_b):
            x = pltpu.bitcast(src[row : row + n].astype(_BF16), _U32)
            kv[0, dst_a + row // 2 : dst_a + (row + n) // 2] = x[:, :H]
            kv[0, dst_b + row // 2 : dst_b + (row + n) // 2] = x[:, H:]

        n_k0 = (_K_FIRST // 2) // RB
        load_k0.wait()
        round_to_bf16(k32, 0, _K_FIRST, 0, HB)
        start_first(0, n_k0)
        load_k1.wait()
        round_to_bf16(k32, _K_FIRST, D - _K_FIRST, 0, HB)
        start_first(n_k0, R // 2)
        load_v.wait()
        round_to_bf16(v32, 0, D, W, HB + W)
        start_first(R // 2, R + 1)

        load_q.wait()
        q16[...] = (q32[...] * scale).T.astype(_BF16)

        ones = jnp.ones((16, H), _BF16)
        on_diagonal = lax.broadcasted_iota(jnp.int32, (H, H), 0) == lax.broadcasted_iota(
            jnp.int32, (H, H), 1
        )

        def column_to_row(col):
            wide = jnp.broadcast_to(col, (H, H))
            return jnp.sum(jnp.where(on_diagonal, wide, 0.0), axis=0, keepdims=True)

        def tile(slot, row):
            return pltpu.bitcast(kv[slot, row : row + W], _BF16)

        def scores(k_tiles):
            maxima = []
            for h in range(2):
                keys = jnp.concatenate([tile(*t) for t in k_tiles], axis=1)
                s = jnp.dot(q16[h * H : (h + 1) * H], keys, preferred_element_type=_F32)
                m = jnp.max(jnp.maximum(s[:, :H], s[:, H:]), axis=1, keepdims=True)
                p = jnp.exp2(s - m).astype(_BF16)
                p16[h * (H // 2) : (h + 1) * (H // 2)] = pltpu.bitcast(p, _U32)
                maxima.append(column_to_row(m))
            return maxima

        def weighted_values(h, v_tiles):
            values = jnp.concatenate(
                [jnp.concatenate([tile(*t), ones], axis=0) for t in v_tiles], axis=1
            )
            p = pltpu.bitcast(p16[h * (H // 2) : (h + 1) * (H // 2)], _BF16)
            return lax.dot_general(values, p, _NT, preferred_element_type=_F32)[: D + 8]

        def rescalers(m_run, m_blk):
            m_new = jnp.maximum(m_run, m_blk)
            return m_new, jnp.exp2(m_run - m_new), jnp.exp2(m_blk - m_new)

        def attend(state, k_tiles, v_tiles):
            maxima = scores(k_tiles)
            out = []
            for h in range(2):
                o = weighted_values(h, v_tiles)
                if state is None:
                    out.append((maxima[h], o))
                else:
                    m_new, a, b = rescalers(state[h][0], maxima[h])
                    out.append((m_new, a * state[h][1] + b * o))
            return out

        state = attend(None, [(0, 0), (0, HB)], [(0, W), (0, HB + W)])

        pl.when(me == 0)(lambda: pl.semaphore_wait(ready_sem, 2))
        pl.when((me == 1) | (me == 3))(lambda: pl.semaphore_wait(ready_sem, 1))

        @pl.when(later_right)
        def _():
            for c in to_right:
                c.start()

        @pl.when(later_left)
        def _():
            for c in to_left:
                c.start()

        def diagonal_row(row):
            return (0, HB, W, HB + W)[row // W] + row % W

        arrivals_l = [
            remote(rows(1, j * RB, RB), rows(1, j * RB, RB), left, SEM_L + j) for j in range(R)
        ]
        arrivals_r = [
            remote(rows(2, HB + j * RB, RB), rows(2, HB + j * RB, RB), right, SEM_R + j)
            for j in range(R)
        ]
        n_send[0] -= 2 * R
        forwards = []
        for j in range(R):
            sem = SEM_DK if j < R // 2 else SEM_DV
            arrivals_l[j].wait_recv()
            c = remote(rows(1, j * RB, RB), rows(3, diagonal_row(j * RB), RB), right, sem)
            c.start()
            forwards.append(c)
            arrivals_r[j].wait_recv()
            c = remote(
                rows(2, HB + j * RB, RB), rows(3, diagonal_row(HB + j * RB), RB), left, sem
            )
            c.start()
            forwards.append(c)

        state = attend(state, [(1, 0), (2, HB)], [(1, W), (2, HB + W)])
        arrivals_l[0].__class__
        remote(rows(1, HB, HB), rows(1, HB, HB), left, SEM_L_REST).wait_recv()
        remote(rows(2, 0, HB), rows(2, 0, HB), right, SEM_R_REST).wait_recv()
        n_send[0] -= 2
        state = attend(state, [(1, HB), (2, 0)], [(1, HB + W), (2, W)])
        for c in to_right + to_left:
            c.wait_send()

        diag_k, diag_v = rows(3, 0, HB), rows(3, HB, HB)
        pltpu.make_async_copy(diag_k, diag_k, recv_sems.at[SEM_DK]).wait()
        maxima = scores([(3, 0), (3, W)])
        merged = []
        for h in range(2):
            _, a, b = rescalers(state[h][0], maxima[h])
            merged.append((a * state[h][1], b))
        for c in forwards:
            c.wait_send()
        pltpu.make_async_copy(diag_v, diag_v, recv_sems.at[SEM_DV]).wait()
        for h in range(2):
            o = weighted_values(h, [(3, HB), (3, HB + W)])
            acc, b = merged[h]
            denom = acc[D : D + 1] + b * o[D : D + 1]
            inv = pl.reciprocal(denom, approx=True)
            inv = inv * (2.0 - denom * inv)
            out_ref[:, h * H : (h + 1) * H] = acc[:D] * inv + o[:D] * (b * inv)

    n_copies = 2 * (_N_RELAY + 1) + 2 * _N_RELAY
    out_t = pl.pallas_call(
        body,
        out_shape=jax.ShapeDtypeStruct((D, S), _F32),
        in_specs=[pl.BlockSpec(memory_space=pl.ANY)] * 3,
        out_specs=pl.BlockSpec(memory_space=pltpu.VMEM),
        scratch_shapes=[
            pltpu.VMEM((D, S), _F32),
            pltpu.VMEM((D, S), _F32),
            pltpu.VMEM((D, S), _F32),
            pltpu.VMEM((4, 2 * HB, H), _U32),
            pltpu.VMEM((S, D), _BF16),
            pltpu.VMEM((S // 2, S), _U32),
            pltpu.SemaphoreType.DMA((4,)),
            pltpu.SemaphoreType.DMA((n_copies,)),
            pltpu.SemaphoreType.DMA((2 * _N_RELAY + 4,)),
            pltpu.SemaphoreType.REGULAR,
        ],
        compiler_params=pltpu.CompilerParams(
            collective_id=0, disable_semaphore_checks=True
        ),
    )(q.T, k.T, v.T)
    return out_t.T
```

```python
import jax
import jax.numpy as jnp
from jax import lax
from jax.experimental import pallas as pl
from jax.experimental.pallas import tpu as pltpu

_N_DEV = 4
_MESH = pl.DeviceIdType.MESH
_BF16 = jnp.bfloat16
_F32 = jnp.float32
_U32 = jnp.uint32
_NT = (((1,), (1,)), ((), ()))
_LOG2E = 1.4426950408889634

_N_RELAY = 8
_K_FIRST = 16


def pallas_dist_ring_attn_i_s256_d64_kernel(
    q: jax.Array,
    k: jax.Array,
    v: jax.Array,
):
    S, D = q.shape
    H = S // 2
    W = D // 2
    HB = 2 * W
    RB = HB // _N_RELAY
    scale = _LOG2E / (D**0.5)

    def body(
        qt_hbm, kt_hbm, vt_hbm, out_ref,
        q32, k32, v32, kv, q16, p16,
        load_sems, send_sems, recv_sems, ready_sem,
    ):
        me = lax.axis_index("i")
        right = (me + 1) % _N_DEV
        left = (me + _N_DEV - 1) % _N_DEV

        first_right = me >= 2
        first_left = (me == 1) | (me == 2)
        later_right = jnp.logical_not(first_right)
        later_left = jnp.logical_not(first_left)

        def signal(sem, target):
            pl.semaphore_signal(sem, inc=1, device_id=(target,), device_id_type=_MESH)

        barrier = pltpu.get_barrier_semaphore()
        pl.when(later_right)(lambda: signal(barrier, right))
        pl.when(later_left)(lambda: signal(barrier, left))

        load_k0 = pltpu.make_async_copy(
            kt_hbm.at[pl.ds(0, _K_FIRST)], k32.at[pl.ds(0, _K_FIRST)], load_sems.at[0]
        )
        load_k1 = pltpu.make_async_copy(
            kt_hbm.at[pl.ds(_K_FIRST, D - _K_FIRST)],
            k32.at[pl.ds(_K_FIRST, D - _K_FIRST)],
            load_sems.at[1],
        )
        load_v = pltpu.make_async_copy(vt_hbm, v32, load_sems.at[2])
        load_q = pltpu.make_async_copy(qt_hbm, q32, load_sems.at[3])
        load_k0.start()
        load_k1.start()
        load_v.start()
        load_q.start()

        pl.when(me == 2)(lambda: pl.semaphore_wait(barrier, 2))
        pl.when((me == 1) | (me == 3))(lambda: pl.semaphore_wait(barrier, 1))
        pl.when(first_left)(lambda: signal(ready_sem, left))
        pl.when(first_right)(lambda: signal(ready_sem, right))

        def rows(slot, start, size):
            return kv.at[slot, pl.ds(start, size)]

        n_send = [0]

        def remote(src, dst, target, recv_sem):
            i = n_send[0]
            n_send[0] += 1
            return pltpu.make_async_remote_copy(
                src_ref=src,
                dst_ref=dst,
                send_sem=send_sems.at[i],
                recv_sem=recv_sems.at[recv_sem],
                device_id=(target,),
                device_id_type=_MESH,
            )

        def wait_arrival(dst, recv_sem):
            pltpu.make_async_remote_copy(
                src_ref=dst,
                dst_ref=dst,
                send_sem=send_sems.at[0],
                recv_sem=recv_sems.at[recv_sem],
                device_id=(me,),
                device_id_type=_MESH,
            ).wait_recv()

        R = _N_RELAY
        SEM_L, SEM_R, SEM_L_REST, SEM_R_REST, SEM_DK, SEM_DV = (
            0, R, 2 * R, 2 * R + 1, 2 * R + 2, 2 * R + 3,
        )
        to_right = [
            remote(rows(0, j * RB, RB), rows(1, j * RB, RB), right, SEM_L + j)
            for j in range(R)
        ] + [remote(rows(0, HB, HB), rows(1, HB, HB), right, SEM_L_REST)]
        to_left = [
            remote(rows(0, HB + j * RB, RB), rows(2, HB + j * RB, RB), left, SEM_R + j)
            for j in range(R)
        ] + [remote(rows(0, 0, HB), rows(2, 0, HB), left, SEM_R_REST)]

        def start_first(lo, hi):
            @pl.when(first_right)
            def _():
                for c in to_right[lo:hi]:
                    c.start()

            @pl.when(first_left)
            def _():
                for c in to_left[lo:hi]:
                    c.start()

        def round_to_bf16(src, row, n, dst_a, dst_b):
            x = pltpu.bitcast(src[row : row + n].astype(_BF16), _U32)
            kv[0, dst_a + row // 2 : dst_a + (row + n) // 2] = x[:, :H]
            kv[0, dst_b + row // 2 : dst_b + (row + n) // 2] = x[:, H:]

        n_k0 = (_K_FIRST // 2) // RB
        load_k0.wait()
        round_to_bf16(k32, 0, _K_FIRST, 0, HB)
        start_first(0, n_k0)
        load_k1.wait()
        round_to_bf16(k32, _K_FIRST, D - _K_FIRST, 0, HB)
        start_first(n_k0, R // 2)
        load_v.wait()
        round_to_bf16(v32, 0, D, W, HB + W)
        start_first(R // 2, R + 1)

        load_q.wait()
        q16[...] = (q32[...] * scale).T.astype(_BF16)

        ones = jnp.ones((16, H), _BF16)
        on_diagonal = lax.broadcasted_iota(jnp.int32, (H, H), 0) == lax.broadcasted_iota(
            jnp.int32, (H, H), 1
        )

        def column_to_row(col):
            wide = jnp.broadcast_to(col, (H, H))
            return jnp.sum(jnp.where(on_diagonal, wide, 0.0), axis=0, keepdims=True)

        def tile(slot, row):
            return pltpu.bitcast(kv[slot, row : row + W], _BF16)

        def scores(k_tiles):
            maxima = []
            for h in range(2):
                keys = jnp.concatenate([tile(*t) for t in k_tiles], axis=1)
                s = jnp.dot(q16[h * H : (h + 1) * H], keys, preferred_element_type=_F32)
                m = jnp.max(jnp.maximum(s[:, :H], s[:, H:]), axis=1, keepdims=True)
                p = jnp.exp2(s - m).astype(_BF16)
                p16[h * (H // 2) : (h + 1) * (H // 2)] = pltpu.bitcast(p, _U32)
                maxima.append(column_to_row(m))
            return maxima

        def weighted_values(h, v_tiles):
            values = jnp.concatenate(
                [jnp.concatenate([tile(*t), ones], axis=0) for t in v_tiles], axis=1
            )
            p = pltpu.bitcast(p16[h * (H // 2) : (h + 1) * (H // 2)], _BF16)
            return lax.dot_general(values, p, _NT, preferred_element_type=_F32)[: D + 8]

        def rescalers(m_run, m_blk):
            m_new = jnp.maximum(m_run, m_blk)
            return m_new, jnp.exp2(m_run - m_new), jnp.exp2(m_blk - m_new)

        def attend(state, k_tiles, v_tiles):
            maxima = scores(k_tiles)
            out = []
            for h in range(2):
                o = weighted_values(h, v_tiles)
                if state is None:
                    out.append((maxima[h], o))
                else:
                    m_new, a, b = rescalers(state[h][0], maxima[h])
                    out.append((m_new, a * state[h][1] + b * o))
            return out

        state = attend(None, [(0, 0), (0, HB)], [(0, W), (0, HB + W)])

        pl.when(me == 0)(lambda: pl.semaphore_wait(ready_sem, 2))
        pl.when((me == 1) | (me == 3))(lambda: pl.semaphore_wait(ready_sem, 1))

        @pl.when(later_right)
        def _():
            for c in to_right:
                c.start()

        @pl.when(later_left)
        def _():
            for c in to_left:
                c.start()

        def diagonal_row(row):
            return (0, HB, W, HB + W)[row // W] + row % W

        forwards = []
        for j in range(R):
            sem = SEM_DK if j < R // 2 else SEM_DV
            wait_arrival(rows(1, j * RB, RB), SEM_L + j)
            c = remote(rows(1, j * RB, RB), rows(3, diagonal_row(j * RB), RB), right, sem)
            c.start()
            forwards.append(c)
            wait_arrival(rows(2, HB + j * RB, RB), SEM_R + j)
            c = remote(
                rows(2, HB + j * RB, RB), rows(3, diagonal_row(HB + j * RB), RB), left, sem
            )
            c.start()
            forwards.append(c)

        state = attend(state, [(1, 0), (2, HB)], [(1, W), (2, HB + W)])
        wait_arrival(rows(1, HB, HB), SEM_L_REST)
        wait_arrival(rows(2, 0, HB), SEM_R_REST)
        state = attend(state, [(1, HB), (2, 0)], [(1, HB + W), (2, W)])
        for c in to_right + to_left:
            c.wait_send()

        diag_k, diag_v = rows(3, 0, HB), rows(3, HB, HB)
        pltpu.make_async_copy(diag_k, diag_k, recv_sems.at[SEM_DK]).wait()
        maxima = scores([(3, 0), (3, W)])
        merged = []
        for h in range(2):
            _, a, b = rescalers(state[h][0], maxima[h])
            merged.append((a * state[h][1], b))
        for c in forwards:
            c.wait_send()
        pltpu.make_async_copy(diag_v, diag_v, recv_sems.at[SEM_DV]).wait()
        for h in range(2):
            o = weighted_values(h, [(3, HB), (3, HB + W)])
            acc, b = merged[h]
            denom = acc[D : D + 1] + b * o[D : D + 1]
            inv = pl.reciprocal(denom, approx=True)
            inv = inv * (2.0 - denom * inv)
            out_ref[:, h * H : (h + 1) * H] = acc[:D] * inv + o[:D] * (b * inv)

    n_copies = 2 * (_N_RELAY + 1) + 2 * _N_RELAY
    out_t = pl.pallas_call(
        body,
        out_shape=jax.ShapeDtypeStruct((D, S), _F32),
        in_specs=[pl.BlockSpec(memory_space=pl.ANY)] * 3,
        out_specs=pl.BlockSpec(memory_space=pltpu.VMEM),
        scratch_shapes=[
            pltpu.VMEM((D, S), _F32),
            pltpu.VMEM((D, S), _F32),
            pltpu.VMEM((D, S), _F32),
            pltpu.VMEM((4, 2 * HB, H), _U32),
            pltpu.VMEM((S, D), _BF16),
            pltpu.VMEM((S // 2, S), _U32),
            pltpu.SemaphoreType.DMA((4,)),
            pltpu.SemaphoreType.DMA((n_copies,)),
            pltpu.SemaphoreType.DMA((2 * _N_RELAY + 4,)),
            pltpu.SemaphoreType.REGULAR,
        ],
        compiler_params=pltpu.CompilerParams(
            collective_id=0, disable_semaphore_checks=True
        ),
    )(q.T, k.T, v.T)
    return out_t.T
```

```python
import jax
import jax.numpy as jnp
from jax import lax
from jax.experimental import pallas as pl
from jax.experimental.pallas import tpu as pltpu

_N_DEV = 4
_MESH = pl.DeviceIdType.MESH
_BF16 = jnp.bfloat16
_F32 = jnp.float32
_U32 = jnp.uint32
_NT = (((1,), (1,)), ((), ()))
_LOG2E = 1.4426950408889634

_N_PIECES = 16
_K_FIRST = 16


def pallas_dist_ring_attn_i_s256_d64_kernel(
    q: jax.Array,
    k: jax.Array,
    v: jax.Array,
):
    S, D = q.shape
    H = S // 2
    W = D // 2
    HB = 2 * W
    R = _N_PIECES
    RB = HB // R
    scale = _LOG2E / (D**0.5)

    def body(
        qt_hbm, kt_hbm, vt_hbm, out_ref,
        q32, k32, v32, kv, q16, p16,
        load_sems, send_sem, recv_sems, ready_sem,
    ):
        me = lax.axis_index("i")
        right = (me + 1) % _N_DEV
        left = (me + _N_DEV - 1) % _N_DEV

        first_right = me >= 2
        first_left = (me == 1) | (me == 2)
        later_right = jnp.logical_not(first_right)
        later_left = jnp.logical_not(first_left)

        def signal(sem, target):
            pl.semaphore_signal(sem, inc=1, device_id=(target,), device_id_type=_MESH)

        barrier = pltpu.get_barrier_semaphore()
        pl.when(later_right)(lambda: signal(barrier, right))
        pl.when(later_left)(lambda: signal(barrier, left))

        load_k0 = pltpu.make_async_copy(
            kt_hbm.at[pl.ds(0, _K_FIRST)], k32.at[pl.ds(0, _K_FIRST)], load_sems.at[0]
        )
        load_k1 = pltpu.make_async_copy(
            kt_hbm.at[pl.ds(_K_FIRST, D - _K_FIRST)],
            k32.at[pl.ds(_K_FIRST, D - _K_FIRST)],
            load_sems.at[1],
        )
        load_v = pltpu.make_async_copy(vt_hbm, v32, load_sems.at[2])
        load_q = pltpu.make_async_copy(qt_hbm, q32, load_sems.at[3])
        load_k0.start()
        load_k1.start()
        load_v.start()
        load_q.start()

        pl.when(me == 2)(lambda: pl.semaphore_wait(barrier, 2))
        pl.when((me == 1) | (me == 3))(lambda: pl.semaphore_wait(barrier, 1))
        pl.when(first_left)(lambda: signal(ready_sem, left))
        pl.when(first_right)(lambda: signal(ready_sem, right))

        def rows(slot, start, size):
            return kv.at[slot, pl.ds(start, size)]

        def remote(src, dst, target, recv_sem):
            return pltpu.make_async_remote_copy(
                src_ref=src,
                dst_ref=dst,
                send_sem=send_sem,
                recv_sem=recv_sems.at[recv_sem],
                device_id=(target,),
                device_id_type=_MESH,
            )

        def wait_arrival(dst, recv_sem):
            remote(dst, dst, me, recv_sem).wait_recv()

        def wait_all_arrivals(dst, recv_sem):
            pltpu.make_async_copy(dst, dst, recv_sems.at[recv_sem]).wait()

        SEM_L, SEM_R = 0, R
        SEM_L_REST, SEM_R_REST, SEM_DIAG_K, SEM_DIAG_V = range(2 * R, 2 * R + 4)
        to_right = [
            remote(rows(0, j * RB, RB), rows(1, j * RB, RB), right, SEM_L + j)
            for j in range(R)
        ] + [remote(rows(0, HB, HB), rows(1, HB, HB), right, SEM_L_REST)]
        to_left = [
            remote(rows(0, HB + j * RB, RB), rows(2, HB + j * RB, RB), left, SEM_R + j)
            for j in range(R)
        ] + [remote(rows(0, 0, HB), rows(2, 0, HB), left, SEM_R_REST)]

        def start_first(lo, hi):
            @pl.when(first_right)
            def _():
                for c in to_right[lo:hi]:
                    c.start()

            @pl.when(first_left)
            def _():
                for c in to_left[lo:hi]:
                    c.start()

        def round_to_bf16(src, row, n, dst_a, dst_b):
            x = pltpu.bitcast(src[row : row + n].astype(_BF16), _U32)
            kv[0, dst_a + row // 2 : dst_a + (row + n) // 2] = x[:, :H]
            kv[0, dst_b + row // 2 : dst_b + (row + n) // 2] = x[:, H:]

        n_first = (_K_FIRST // 2) // RB
        load_k0.wait()
        round_to_bf16(k32, 0, _K_FIRST, 0, HB)
        start_first(0, n_first)
        load_k1.wait()
        round_to_bf16(k32, _K_FIRST, D - _K_FIRST, 0, HB)
        start_first(n_first, R // 2)
        load_v.wait()
        round_to_bf16(v32, 0, D, W, HB + W)
        start_first(R // 2, R + 1)

        load_q.wait()
        q16[...] = pltpu.bitcast((q32[...] * scale).T.astype(_BF16), _U32)

        ones = jnp.ones((16, H), _BF16)
        on_diagonal = lax.broadcasted_iota(jnp.int32, (H, H), 0) == lax.broadcasted_iota(
            jnp.int32, (H, H), 1
        )

        def column_to_row(col):
            wide = jnp.broadcast_to(col, (H, H))
            return jnp.sum(jnp.where(on_diagonal, wide, 0.0), axis=0, keepdims=True)

        def tile(slot, row):
            return pltpu.bitcast(kv[slot, row : row + W], _BF16)

        def half(ref, h):
            return pltpu.bitcast(ref[h * (H // 2) : (h + 1) * (H // 2)], _BF16)

        def scores(k_tiles):
            maxima = []
            for h in range(2):
                keys = jnp.concatenate([tile(*t) for t in k_tiles], axis=1)
                s = jnp.dot(half(q16, h), keys, preferred_element_type=_F32)
                m = jnp.max(jnp.maximum(s[:, :H], s[:, H:]), axis=1, keepdims=True)
                p = jnp.exp2(s - m).astype(_BF16)
                p16[h * (H // 2) : (h + 1) * (H // 2)] = pltpu.bitcast(p, _U32)
                maxima.append(column_to_row(m))
            return maxima

        def weighted_values(h, v_tiles):
            values = jnp.concatenate(
                [jnp.concatenate([tile(*t), ones], axis=0) for t in v_tiles], axis=1
            )
            return lax.dot_general(
                values, half(p16, h), _NT, preferred_element_type=_F32
            )[: D + 8]

        def rescalers(m_run, m_blk):
            m_new = jnp.maximum(m_run, m_blk)
            return m_new, jnp.exp2(m_run - m_new), jnp.exp2(m_blk - m_new)

        def attend(state, k_tiles, v_tiles):
            maxima = scores(k_tiles)
            out = []
            for h in range(2):
                o = weighted_values(h, v_tiles)
                if state is None:
                    out.append((maxima[h], o))
                else:
                    m_new, a, b = rescalers(state[h][0], maxima[h])
                    out.append((m_new, a * state[h][1] + b * o))
            return out

        state = attend(None, [(0, 0), (0, HB)], [(0, W), (0, HB + W)])

        pl.when(me == 0)(lambda: pl.semaphore_wait(ready_sem, 2))
        pl.when((me == 1) | (me == 3))(lambda: pl.semaphore_wait(ready_sem, 1))

        @pl.when(later_right)
        def _():
            for c in to_right:
                c.start()

        @pl.when(later_left)
        def _():
            for c in to_left:
                c.start()

        def diagonal_row(row):
            return (0, HB, W, HB + W)[row // W] + row % W

        for j in range(R):
            sem = SEM_DIAG_K if j < R // 2 else SEM_DIAG_V
            src = rows(1, j * RB, RB)
            wait_arrival(src, SEM_L + j)
            remote(src, rows(3, diagonal_row(j * RB), RB), right, sem).start()
            src = rows(2, HB + j * RB, RB)
            wait_arrival(src, SEM_R + j)
            remote(src, rows(3, diagonal_row(HB + j * RB), RB), left, sem).start()

        state = attend(state, [(1, 0), (2, HB)], [(1, W), (2, HB + W)])
        wait_arrival(rows(1, HB, HB), SEM_L_REST)
        wait_arrival(rows(2, 0, HB), SEM_R_REST)
        state = attend(state, [(1, HB), (2, 0)], [(1, HB + W), (2, W)])

        wait_all_arrivals(rows(3, 0, HB), SEM_DIAG_K)
        maxima = scores([(3, 0), (3, W)])
        merged = []
        for h in range(2):
            _, a, b = rescalers(state[h][0], maxima[h])
            merged.append((a * state[h][1], b))
        sent = kv.at[pl.ds(0, 3)]
        pltpu.make_async_copy(sent, sent, send_sem).wait()
        wait_all_arrivals(rows(3, HB, HB), SEM_DIAG_V)
        for h in range(2):
            o = weighted_values(h, [(3, HB), (3, HB + W)])
            acc, b = merged[h]
            denom = acc[D : D + 1] + b * o[D : D + 1]
            inv = pl.reciprocal(denom, approx=True)
            inv = inv * (2.0 - denom * inv)
            out_ref[:, h * H : (h + 1) * H] = acc[:D] * inv + o[:D] * (b * inv)

    out_t = pl.pallas_call(
        body,
        out_shape=jax.ShapeDtypeStruct((D, S), _F32),
        in_specs=[pl.BlockSpec(memory_space=pl.ANY)] * 3,
        out_specs=pl.BlockSpec(memory_space=pltpu.VMEM),
        scratch_shapes=[
            pltpu.VMEM((D, S), _F32),
            pltpu.VMEM((D, S), _F32),
            pltpu.VMEM((D, S), _F32),
            pltpu.VMEM((4, 2 * HB, H), _U32),
            pltpu.VMEM((S // 2, D), _U32),
            pltpu.VMEM((S // 2, S), _U32),
            pltpu.SemaphoreType.DMA((4,)),
            pltpu.SemaphoreType.DMA,
            pltpu.SemaphoreType.DMA((2 * _N_PIECES + 4,)),
            pltpu.SemaphoreType.REGULAR,
        ],
        compiler_params=pltpu.CompilerParams(
            collective_id=0, disable_semaphore_checks=True
        ),
    )(q.T, k.T, v.T)
    return out_t.T
```

```python
import jax
import jax.numpy as jnp
from jax import lax
from jax.experimental import pallas as pl
from jax.experimental.pallas import tpu as pltpu

_N_DEV = 4
_MESH = pl.DeviceIdType.MESH
_BF16 = jnp.bfloat16
_F32 = jnp.float32
_U32 = jnp.uint32
_NT = (((1,), (1,)), ((), ()))
_LOG2E = 1.4426950408889634

_N_PIECES = 16
_K_FIRST = 16


def pallas_dist_ring_attn_i_s256_d64_kernel(
    q: jax.Array,
    k: jax.Array,
    v: jax.Array,
):
    S, D = q.shape
    H = S // 2
    W = D // 2
    HB = 2 * W
    R = _N_PIECES
    RB = HB // R
    scale = _LOG2E / (D**0.5)

    def ring_attention(
        qt_hbm, kt_hbm, vt_hbm, out_ref,
        q32, k32, v32, kv, q16, p16,
        load_sems, send_sem, recv_sems, ready_sem,
    ):
        me = lax.axis_index("i")
        right = (me + 1) % _N_DEV
        left = (me + _N_DEV - 1) % _N_DEV

        first_right = me >= 2
        first_left = (me == 1) | (me == 2)
        later_right = jnp.logical_not(first_right)
        later_left = jnp.logical_not(first_left)

        def signal(sem, target):
            pl.semaphore_signal(sem, inc=1, device_id=(target,), device_id_type=_MESH)

        barrier = pltpu.get_barrier_semaphore()
        pl.when(later_right)(lambda: signal(barrier, right))
        pl.when(later_left)(lambda: signal(barrier, left))

        load_k0 = pltpu.make_async_copy(
            kt_hbm.at[pl.ds(0, _K_FIRST)], k32.at[pl.ds(0, _K_FIRST)], load_sems.at[0]
        )
        load_k1 = pltpu.make_async_copy(
            kt_hbm.at[pl.ds(_K_FIRST, D - _K_FIRST)],
            k32.at[pl.ds(_K_FIRST, D - _K_FIRST)],
            load_sems.at[1],
        )
        load_v = pltpu.make_async_copy(vt_hbm, v32, load_sems.at[2])
        load_q = pltpu.make_async_copy(qt_hbm, q32, load_sems.at[3])
        load_k0.start()
        load_k1.start()
        load_v.start()
        load_q.start()

        pl.when(me == 2)(lambda: pl.semaphore_wait(barrier, 2))
        pl.when((me == 1) | (me == 3))(lambda: pl.semaphore_wait(barrier, 1))
        pl.when(first_left)(lambda: signal(ready_sem, left))
        pl.when(first_right)(lambda: signal(ready_sem, right))

        def rows(slot, start, size):
            return kv.at[slot, pl.ds(start, size)]

        def remote(src, dst, target, recv_sem):
            return pltpu.make_async_remote_copy(
                src_ref=src,
                dst_ref=dst,
                send_sem=send_sem,
                recv_sem=recv_sems.at[recv_sem],
                device_id=(target,),
                device_id_type=_MESH,
            )

        def wait_arrival(dst, recv_sem):
            remote(dst, dst, me, recv_sem).wait_recv()

        def wait_all_arrivals(dst, recv_sem):
            pltpu.make_async_copy(dst, dst, recv_sems.at[recv_sem]).wait()

        SEM_L, SEM_R = 0, R
        SEM_L_REST, SEM_R_REST, SEM_DIAG_K, SEM_DIAG_V = range(2 * R, 2 * R + 4)
        to_right = [
            remote(rows(0, j * RB, RB), rows(1, j * RB, RB), right, SEM_L + j)
            for j in range(R)
        ] + [remote(rows(0, HB, HB), rows(1, HB, HB), right, SEM_L_REST)]
        to_left = [
            remote(rows(0, HB + j * RB, RB), rows(2, HB + j * RB, RB), left, SEM_R + j)
            for j in range(R)
        ] + [remote(rows(0, 0, HB), rows(2, 0, HB), left, SEM_R_REST)]

        def start_first(lo, hi):
            @pl.when(first_right)
            def _():
                for c in to_right[lo:hi]:
                    c.start()

            @pl.when(first_left)
            def _():
                for c in to_left[lo:hi]:
                    c.start()

        def round_to_bf16(src, row, n, dst_a, dst_b):
            x = pltpu.bitcast(src[row : row + n].astype(_BF16), _U32)
            kv[0, dst_a + row // 2 : dst_a + (row + n) // 2] = x[:, :H]
            kv[0, dst_b + row // 2 : dst_b + (row + n) // 2] = x[:, H:]

        n_first = (_K_FIRST // 2) // RB
        load_k0.wait()
        round_to_bf16(k32, 0, _K_FIRST, 0, HB)
        start_first(0, n_first)
        load_k1.wait()
        round_to_bf16(k32, _K_FIRST, D - _K_FIRST, 0, HB)
        start_first(n_first, R // 2)
        load_v.wait()
        round_to_bf16(v32, 0, D, W, HB + W)
        start_first(R // 2, R + 1)

        load_q.wait()
        q16[...] = pltpu.bitcast((q32[...] * scale).T.astype(_BF16), _U32)

        ones = jnp.ones((16, H), _BF16)
        on_diagonal = lax.broadcasted_iota(jnp.int32, (H, H), 0) == lax.broadcasted_iota(
            jnp.int32, (H, H), 1
        )

        def column_to_row(col):
            wide = jnp.broadcast_to(col, (H, H))
            return jnp.sum(jnp.where(on_diagonal, wide, 0.0), axis=0, keepdims=True)

        def tile(slot, row):
            return pltpu.bitcast(kv[slot, row : row + W], _BF16)

        def half(ref, h):
            return pltpu.bitcast(ref[h * (H // 2) : (h + 1) * (H // 2)], _BF16)

        def scores(k_tiles):
            maxima = []
            for h in range(2):
                keys = jnp.concatenate([tile(*t) for t in k_tiles], axis=1)
                s = jnp.dot(half(q16, h), keys, preferred_element_type=_F32)
                m = jnp.max(jnp.maximum(s[:, :H], s[:, H:]), axis=1, keepdims=True)
                p = jnp.exp2(s - m).astype(_BF16)
                p16[h * (H // 2) : (h + 1) * (H // 2)] = pltpu.bitcast(p, _U32)
                maxima.append(column_to_row(m))
            return maxima

        def weighted_values(h, v_tiles):
            values = jnp.concatenate(
                [jnp.concatenate([tile(*t), ones], axis=0) for t in v_tiles], axis=1
            )
            return lax.dot_general(
                values, half(p16, h), _NT, preferred_element_type=_F32
            )[: D + 8]

        def rescalers(m_run, m_blk):
            m_new = jnp.maximum(m_run, m_blk)
            return m_new, jnp.exp2(m_run - m_new), jnp.exp2(m_blk - m_new)

        def attend(state, k_tiles, v_tiles):
            maxima = scores(k_tiles)
            out = []
            for h in range(2):
                o = weighted_values(h, v_tiles)
                if state is None:
                    out.append((maxima[h], o))
                else:
                    m_new, a, b = rescalers(state[h][0], maxima[h])
                    out.append((m_new, a * state[h][1] + b * o))
            return out

        state = attend(None, [(0, 0), (0, HB)], [(0, W), (0, HB + W)])

        pl.when(me == 0)(lambda: pl.semaphore_wait(ready_sem, 2))
        pl.when((me == 1) | (me == 3))(lambda: pl.semaphore_wait(ready_sem, 1))

        @pl.when(later_right)
        def _():
            for c in to_right:
                c.start()

        @pl.when(later_left)
        def _():
            for c in to_left:
                c.start()

        def diagonal_row(row):
            return (0, HB, W, HB + W)[row // W] + row % W

        for j in range(R):
            sem = SEM_DIAG_K if j < R // 2 else SEM_DIAG_V
            src = rows(1, j * RB, RB)
            wait_arrival(src, SEM_L + j)
            remote(src, rows(3, diagonal_row(j * RB), RB), right, sem).start()
            src = rows(2, HB + j * RB, RB)
            wait_arrival(src, SEM_R + j)
            remote(src, rows(3, diagonal_row(HB + j * RB), RB), left, sem).start()

        state = attend(state, [(1, 0), (2, HB)], [(1, W), (2, HB + W)])
        wait_arrival(rows(1, HB, HB), SEM_L_REST)
        wait_arrival(rows(2, 0, HB), SEM_R_REST)
        state = attend(state, [(1, HB), (2, 0)], [(1, HB + W), (2, W)])

        wait_all_arrivals(rows(3, 0, HB), SEM_DIAG_K)
        maxima = scores([(3, 0), (3, W)])
        merged = []
        for h in range(2):
            _, a, b = rescalers(state[h][0], maxima[h])
            merged.append((a * state[h][1], b))
        sent = kv.at[pl.ds(0, 3)]
        pltpu.make_async_copy(sent, sent, send_sem).wait()
        wait_all_arrivals(rows(3, HB, HB), SEM_DIAG_V)
        for h in range(2):
            o = weighted_values(h, [(3, HB), (3, HB + W)])
            acc, b = merged[h]
            denom = acc[D : D + 1] + b * o[D : D + 1]
            inv = pl.reciprocal(denom, approx=True)
            inv = inv * (2.0 - denom * inv)
            out_ref[:, h * H : (h + 1) * H] = acc[:D] * inv + o[:D] * (b * inv)

    def body(*refs):
        pl.run_scoped(
            lambda *sems: ring_attention(*refs, *sems),
            pltpu.SemaphoreType.DMA((4,)),
            pltpu.SemaphoreType.DMA(()),
            pltpu.SemaphoreType.DMA((2 * _N_PIECES + 4,)),
            pltpu.SemaphoreType.REGULAR(()),
        )

    out_t = pl.pallas_call(
        body,
        out_shape=jax.ShapeDtypeStruct((D, S), _F32),
        in_specs=[pl.BlockSpec(memory_space=pl.ANY)] * 3,
        out_specs=pl.BlockSpec(memory_space=pltpu.VMEM),
        scratch_shapes=[
            pltpu.VMEM((D, S), _F32),
            pltpu.VMEM((D, S), _F32),
            pltpu.VMEM((D, S), _F32),
            pltpu.VMEM((4, 2 * HB, H), _U32),
            pltpu.VMEM((S // 2, D), _U32),
            pltpu.VMEM((S // 2, S), _U32),
        ],
        compiler_params=pltpu.CompilerParams(collective_id=0),
    )(q.T, k.T, v.T)
    return out_t.T
```

```python
import jax
import jax.numpy as jnp
from jax import lax
from jax.experimental import pallas as pl
from jax.experimental.pallas import tpu as pltpu

_N_DEV = 4
_MESH = pl.DeviceIdType.MESH
_BF16 = jnp.bfloat16
_F32 = jnp.float32
_NT = (((1,), (1,)), ((), ()))
_LOG2E = 1.4426950408889634

_N_PIECES = 16
_K_FIRST = 16


def pallas_dist_ring_attn_i_s256_d64_kernel(
    q: jax.Array,
    k: jax.Array,
    v: jax.Array,
):
    S, D = q.shape
    H = S // 2
    W = D
    HB = 2 * W
    R = _N_PIECES
    RB = HB // R
    scale = _LOG2E / (D**0.5)

    def ring_attention(
        qt_hbm, kt_hbm, vt_hbm, out_ref,
        q32, k32, v32, kv, q16, p16,
        load_sems, send_sem, recv_sems, ready_sem,
    ):
        me = lax.axis_index("i")
        right = (me + 1) % _N_DEV
        left = (me + _N_DEV - 1) % _N_DEV

        first_right = me >= 2
        first_left = (me == 1) | (me == 2)
        later_right = jnp.logical_not(first_right)
        later_left = jnp.logical_not(first_left)

        def signal(sem, target):
            pl.semaphore_signal(sem, inc=1, device_id=(target,), device_id_type=_MESH)

        barrier = pltpu.get_barrier_semaphore()
        pl.when(later_right)(lambda: signal(barrier, right))
        pl.when(later_left)(lambda: signal(barrier, left))

        load_k0 = pltpu.make_async_copy(
            kt_hbm.at[pl.ds(0, _K_FIRST)], k32.at[pl.ds(0, _K_FIRST)], load_sems.at[0]
        )
        load_k1 = pltpu.make_async_copy(
            kt_hbm.at[pl.ds(_K_FIRST, D - _K_FIRST)],
            k32.at[pl.ds(_K_FIRST, D - _K_FIRST)],
            load_sems.at[1],
        )
        load_v = pltpu.make_async_copy(vt_hbm, v32, load_sems.at[2])
        load_q = pltpu.make_async_copy(qt_hbm, q32, load_sems.at[3])
        load_k0.start()
        load_k1.start()
        load_v.start()
        load_q.start()

        pl.when(me == 2)(lambda: pl.semaphore_wait(barrier, 2))
        pl.when((me == 1) | (me == 3))(lambda: pl.semaphore_wait(barrier, 1))
        pl.when(first_left)(lambda: signal(ready_sem, left))
        pl.when(first_right)(lambda: signal(ready_sem, right))

        def rows(slot, start, size):
            return kv.at[slot, pl.ds(start, size)]

        def remote(src, dst, target, recv_sem):
            return pltpu.make_async_remote_copy(
                src_ref=src,
                dst_ref=dst,
                send_sem=send_sem,
                recv_sem=recv_sems.at[recv_sem],
                device_id=(target,),
                device_id_type=_MESH,
            )

        def wait_arrival(dst, recv_sem):
            remote(dst, dst, me, recv_sem).wait_recv()

        def wait_all_arrivals(dst, recv_sem):
            pltpu.make_async_copy(dst, dst, recv_sems.at[recv_sem]).wait()

        SEM_L, SEM_R = 0, R
        SEM_L_REST, SEM_R_REST, SEM_DIAG_K, SEM_DIAG_V = range(2 * R, 2 * R + 4)
        to_right = [
            remote(rows(0, j * RB, RB), rows(1, j * RB, RB), right, SEM_L + j)
            for j in range(R)
        ] + [remote(rows(0, HB, HB), rows(1, HB, HB), right, SEM_L_REST)]
        to_left = [
            remote(rows(0, HB + j * RB, RB), rows(2, HB + j * RB, RB), left, SEM_R + j)
            for j in range(R)
        ] + [remote(rows(0, 0, HB), rows(2, 0, HB), left, SEM_R_REST)]

        def start_first(lo, hi):
            @pl.when(first_right)
            def _():
                for c in to_right[lo:hi]:
                    c.start()

            @pl.when(first_left)
            def _():
                for c in to_left[lo:hi]:
                    c.start()

        def round_to_bf16(src, row, n, dst_a, dst_b):
            x = src[row : row + n].astype(_BF16)
            kv[0, dst_a + row : dst_a + row + n] = x[:, :H]
            kv[0, dst_b + row : dst_b + row + n] = x[:, H:]

        n_first = _K_FIRST // RB
        load_k0.wait()
        round_to_bf16(k32, 0, _K_FIRST, 0, HB)
        start_first(0, n_first)
        load_k1.wait()
        round_to_bf16(k32, _K_FIRST, D - _K_FIRST, 0, HB)
        start_first(n_first, R // 2)
        load_v.wait()
        round_to_bf16(v32, 0, D, W, HB + W)
        start_first(R // 2, R + 1)

        load_q.wait()
        q16[...] = (q32[...] * scale).T.astype(_BF16)

        ones = jnp.ones((16, H), _BF16)
        on_diagonal = lax.broadcasted_iota(jnp.int32, (H, H), 0) == lax.broadcasted_iota(
            jnp.int32, (H, H), 1
        )

        def column_to_row(col):
            wide = jnp.broadcast_to(col, (H, H))
            return jnp.sum(jnp.where(on_diagonal, wide, 0.0), axis=0, keepdims=True)

        def tile(slot, row):
            return kv[slot, row : row + W]

        def half(ref, h):
            return ref[h * H : (h + 1) * H]

        def scores(k_tiles):
            maxima = []
            for h in range(2):
                keys = jnp.concatenate([tile(*t) for t in k_tiles], axis=1)
                s = jnp.dot(half(q16, h), keys, preferred_element_type=_F32)
                m = jnp.max(jnp.maximum(s[:, :H], s[:, H:]), axis=1, keepdims=True)
                p = jnp.exp2(s - m).astype(_BF16)
                p16[h * H : (h + 1) * H] = p
                maxima.append(column_to_row(m))
            return maxima

        def weighted_values(h, v_tiles):
            values = jnp.concatenate(
                [jnp.concatenate([tile(*t), ones], axis=0) for t in v_tiles], axis=1
            )
            return lax.dot_general(
                values, half(p16, h), _NT, preferred_element_type=_F32
            )[: D + 8]

        def rescalers(m_run, m_blk):
            m_new = jnp.maximum(m_run, m_blk)
            return m_new, jnp.exp2(m_run - m_new), jnp.exp2(m_blk - m_new)

        def attend(state, k_tiles, v_tiles):
            maxima = scores(k_tiles)
            out = []
            for h in range(2):
                o = weighted_values(h, v_tiles)
                if state is None:
                    out.append((maxima[h], o))
                else:
                    m_new, a, b = rescalers(state[h][0], maxima[h])
                    out.append((m_new, a * state[h][1] + b * o))
            return out

        state = attend(None, [(0, 0), (0, HB)], [(0, W), (0, HB + W)])

        pl.when(me == 0)(lambda: pl.semaphore_wait(ready_sem, 2))
        pl.when((me == 1) | (me == 3))(lambda: pl.semaphore_wait(ready_sem, 1))

        @pl.when(later_right)
        def _():
            for c in to_right:
                c.start()

        @pl.when(later_left)
        def _():
            for c in to_left:
                c.start()

        def diagonal_row(row):
            return (0, HB, W, HB + W)[row // W] + row % W

        for j in range(R):
            sem = SEM_DIAG_K if j < R // 2 else SEM_DIAG_V
            src = rows(1, j * RB, RB)
            wait_arrival(src, SEM_L + j)
            remote(src, rows(3, diagonal_row(j * RB), RB), right, sem).start()
            src = rows(2, HB + j * RB, RB)
            wait_arrival(src, SEM_R + j)
            remote(src, rows(3, diagonal_row(HB + j * RB), RB), left, sem).start()

        state = attend(state, [(1, 0), (2, HB)], [(1, W), (2, HB + W)])
        wait_arrival(rows(1, HB, HB), SEM_L_REST)
        wait_arrival(rows(2, 0, HB), SEM_R_REST)
        state = attend(state, [(1, HB), (2, 0)], [(1, HB + W), (2, W)])

        wait_all_arrivals(rows(3, 0, HB), SEM_DIAG_K)
        maxima = scores([(3, 0), (3, W)])
        merged = []
        for h in range(2):
            _, a, b = rescalers(state[h][0], maxima[h])
            merged.append((a * state[h][1], b))
        sent = kv.at[pl.ds(0, 3)]
        pltpu.make_async_copy(sent, sent, send_sem).wait()
        wait_all_arrivals(rows(3, HB, HB), SEM_DIAG_V)
        for h in range(2):
            o = weighted_values(h, [(3, HB), (3, HB + W)])
            acc, b = merged[h]
            denom = acc[D : D + 1] + b * o[D : D + 1]
            inv = pl.reciprocal(denom, approx=True)
            inv = inv * (2.0 - denom * inv)
            out_ref[:, h * H : (h + 1) * H] = acc[:D] * inv + o[:D] * (b * inv)

    def body(*refs):
        pl.run_scoped(
            lambda *sems: ring_attention(*refs, *sems),
            pltpu.SemaphoreType.DMA((4,)),
            pltpu.SemaphoreType.DMA(()),
            pltpu.SemaphoreType.DMA((2 * _N_PIECES + 4,)),
            pltpu.SemaphoreType.REGULAR(()),
        )

    out_t = pl.pallas_call(
        body,
        out_shape=jax.ShapeDtypeStruct((D, S), _F32),
        in_specs=[pl.BlockSpec(memory_space=pl.ANY)] * 3,
        out_specs=pl.BlockSpec(memory_space=pltpu.VMEM),
        scratch_shapes=[
            pltpu.VMEM((D, S), _F32),
            pltpu.VMEM((D, S), _F32),
            pltpu.VMEM((D, S), _F32),
            pltpu.VMEM((4, 2 * HB, H), _BF16),
            pltpu.VMEM((S, D), _BF16),
            pltpu.VMEM((S, S), _BF16),
        ],
        compiler_params=pltpu.CompilerParams(collective_id=0),
    )(q.T, k.T, v.T)
    return out_t.T
```

```python
import jax
import jax.numpy as jnp
from jax import lax
from jax.experimental import pallas as pl
from jax.experimental.pallas import tpu as pltpu

_N_DEV = 4
_MESH = pl.DeviceIdType.MESH
_BF16 = jnp.bfloat16
_F32 = jnp.float32
_NT = (((1,), (1,)), ((), ()))
_LOG2E = 1.4426950408889634

_N_PIECES = 16
_K_FIRST = 16


def pallas_dist_ring_attn_i_s256_d64_kernel(
    q: jax.Array,
    k: jax.Array,
    v: jax.Array,
):
    S, D = q.shape
    H = S // 2
    W = D
    HB = 2 * W
    R = _N_PIECES
    RB = HB // R
    scale = _LOG2E / (D**0.5)

    def ring_attention(
        qt_hbm, kt_hbm, vt_hbm, out_ref,
        q32, k32, v32, kv, q16, p16,
        load_sems, send_sem, recv_sems, ready_sem,
    ):
        me = lax.axis_index("i")
        right = (me + 1) % _N_DEV
        left = (me + _N_DEV - 1) % _N_DEV

        first_right = me >= 2
        first_left = (me == 1) | (me == 2)
        later_right = jnp.logical_not(first_right)
        later_left = jnp.logical_not(first_left)

        def signal(sem, target):
            pl.semaphore_signal(sem, inc=1, device_id=(target,), device_id_type=_MESH)

        barrier = pltpu.get_barrier_semaphore()
        pl.when(later_right)(lambda: signal(barrier, right))
        pl.when(later_left)(lambda: signal(barrier, left))

        load_k0 = pltpu.make_async_copy(
            kt_hbm.at[pl.ds(0, _K_FIRST)], k32.at[pl.ds(0, _K_FIRST)], load_sems.at[0]
        )
        load_k1 = pltpu.make_async_copy(
            kt_hbm.at[pl.ds(_K_FIRST, D - _K_FIRST)],
            k32.at[pl.ds(_K_FIRST, D - _K_FIRST)],
            load_sems.at[1],
        )
        load_v = pltpu.make_async_copy(vt_hbm, v32, load_sems.at[2])
        load_q = pltpu.make_async_copy(qt_hbm, q32, load_sems.at[3])
        load_k0.start()
        load_k1.start()
        load_v.start()
        load_q.start()

        pl.when(me == 2)(lambda: pl.semaphore_wait(barrier, 2))
        pl.when((me == 1) | (me == 3))(lambda: pl.semaphore_wait(barrier, 1))
        pl.when(first_left)(lambda: signal(ready_sem, left))
        pl.when(first_right)(lambda: signal(ready_sem, right))

        def rows(slot, start, size):
            return kv.at[slot, pl.ds(start, size)]

        def remote(src, dst, target, recv_sem):
            return pltpu.make_async_remote_copy(
                src_ref=src,
                dst_ref=dst,
                send_sem=send_sem,
                recv_sem=recv_sems.at[recv_sem],
                device_id=(target,),
                device_id_type=_MESH,
            )

        def wait_arrival(dst, recv_sem):
            remote(dst, dst, me, recv_sem).wait_recv()

        def wait_all_arrivals(dst, recv_sem):
            pltpu.make_async_copy(dst, dst, recv_sems.at[recv_sem]).wait()

        SEM_L, SEM_R = 0, R
        SEM_L_REST, SEM_R_REST, SEM_DIAG_K, SEM_DIAG_V = range(2 * R, 2 * R + 4)
        to_right = [
            remote(rows(0, j * RB, RB), rows(1, j * RB, RB), right, SEM_L + j)
            for j in range(R)
        ] + [remote(rows(0, HB, HB), rows(1, HB, HB), right, SEM_L_REST)]
        to_left = [
            remote(rows(0, HB + j * RB, RB), rows(2, HB + j * RB, RB), left, SEM_R + j)
            for j in range(R)
        ] + [remote(rows(0, 0, HB), rows(2, 0, HB), left, SEM_R_REST)]

        def start_first(lo, hi):
            @pl.when(first_right)
            def _():
                for c in to_right[lo:hi]:
                    c.start()

            @pl.when(first_left)
            def _():
                for c in to_left[lo:hi]:
                    c.start()

        def round_to_bf16(src, row, n, dst_a, dst_b):
            x = src[row : row + n].astype(_BF16)
            kv[0, dst_a + row : dst_a + row + n] = x[:, :H]
            kv[0, dst_b + row : dst_b + row + n] = x[:, H:]

        n_first = _K_FIRST // RB
        load_k0.wait()
        round_to_bf16(k32, 0, _K_FIRST, 0, HB)
        start_first(0, n_first)
        load_k1.wait()
        round_to_bf16(k32, _K_FIRST, D - _K_FIRST, 0, HB)
        start_first(n_first, R // 2)
        load_v.wait()
        round_to_bf16(v32, 0, D, W, HB + W)
        start_first(R // 2, R + 1)

        load_q.wait()
        q16[...] = (q32[...] * scale).T.astype(_BF16)

        ones = jnp.ones((16, H), _BF16)
        on_diagonal = lax.broadcasted_iota(jnp.int32, (H, H), 0) == lax.broadcasted_iota(
            jnp.int32, (H, H), 1
        )

        def column_to_row(col):
            wide = jnp.broadcast_to(col, (H, H))
            return jnp.sum(jnp.where(on_diagonal, wide, 0.0), axis=0, keepdims=True)

        def tile(slot, row):
            return kv[slot, row : row + W]

        def half(ref, h):
            return ref[h * H : (h + 1) * H]

        def scores(k_tiles):
            maxima = []
            for h in range(2):
                keys = jnp.concatenate([tile(*t) for t in k_tiles], axis=1)
                s = jnp.dot(half(q16, h), keys, preferred_element_type=_F32)
                m = jnp.max(jnp.maximum(s[:, :H], s[:, H:]), axis=1, keepdims=True)
                p = jnp.exp2(s - m).astype(_BF16)
                p16[h * H : (h + 1) * H] = p
                maxima.append(column_to_row(m))
            return maxima

        def weighted_values(h, v_tiles):
            values = jnp.concatenate(
                [jnp.concatenate([tile(*t), ones], axis=0) for t in v_tiles], axis=1
            )
            return lax.dot_general(
                values, half(p16, h), _NT, preferred_element_type=_F32
            )[: D + 8]

        def rescalers(m_run, m_blk):
            m_new = jnp.maximum(m_run, m_blk)
            return m_new, jnp.exp2(m_run - m_new), jnp.exp2(m_blk - m_new)

        def attend(state, k_tiles, v_tiles):
            maxima = scores(k_tiles)
            out = []
            for h in range(2):
                o = weighted_values(h, v_tiles)
                if state is None:
                    out.append((maxima[h], o))
                else:
                    m_new, a, b = rescalers(state[h][0], maxima[h])
                    out.append((m_new, a * state[h][1] + b * o))
            return out

        state = attend(None, [(0, 0), (0, HB)], [(0, W), (0, HB + W)])

        pl.when(me == 0)(lambda: pl.semaphore_wait(ready_sem, 2))
        pl.when((me == 1) | (me == 3))(lambda: pl.semaphore_wait(ready_sem, 1))

        @pl.when(later_right)
        def _():
            for c in to_right:
                c.start()

        @pl.when(later_left)
        def _():
            for c in to_left:
                c.start()

        def diagonal_row(row):
            return (0, HB, W, HB + W)[row // W] + row % W

        forwards = []

        def forward(src, row, target, sem):
            c = remote(src, rows(3, diagonal_row(row), RB), target, sem)
            c.start()
            forwards.append(c)

        for j in range(R):
            sem = SEM_DIAG_K if j < R // 2 else SEM_DIAG_V
            src = rows(1, j * RB, RB)
            wait_arrival(src, SEM_L + j)
            forward(src, j * RB, right, sem)
            src = rows(2, HB + j * RB, RB)
            wait_arrival(src, SEM_R + j)
            forward(src, HB + j * RB, left, sem)

        state = attend(state, [(1, 0), (2, HB)], [(1, W), (2, HB + W)])
        wait_arrival(rows(1, HB, HB), SEM_L_REST)
        wait_arrival(rows(2, 0, HB), SEM_R_REST)
        state = attend(state, [(1, HB), (2, 0)], [(1, HB + W), (2, W)])

        for c in to_right + to_left + forwards:
            c.wait_send()

        wait_all_arrivals(rows(3, 0, HB), SEM_DIAG_K)
        maxima = scores([(3, 0), (3, W)])
        merged = []
        for h in range(2):
            _, a, b = rescalers(state[h][0], maxima[h])
            merged.append((a * state[h][1], b))
        wait_all_arrivals(rows(3, HB, HB), SEM_DIAG_V)
        for h in range(2):
            o = weighted_values(h, [(3, HB), (3, HB + W)])
            acc, b = merged[h]
            denom = acc[D : D + 1] + b * o[D : D + 1]
            inv = pl.reciprocal(denom, approx=True)
            inv = inv * (2.0 - denom * inv)
            out_ref[:, h * H : (h + 1) * H] = acc[:D] * inv + o[:D] * (b * inv)

    def body(*refs):
        pl.run_scoped(
            lambda *sems: ring_attention(*refs, *sems),
            pltpu.SemaphoreType.DMA((4,)),
            pltpu.SemaphoreType.DMA(()),
            pltpu.SemaphoreType.DMA((2 * _N_PIECES + 4,)),
            pltpu.SemaphoreType.REGULAR(()),
        )

    out_t = pl.pallas_call(
        body,
        out_shape=jax.ShapeDtypeStruct((D, S), _F32),
        in_specs=[pl.BlockSpec(memory_space=pl.ANY)] * 3,
        out_specs=pl.BlockSpec(memory_space=pltpu.VMEM),
        scratch_shapes=[
            pltpu.VMEM((D, S), _F32),
            pltpu.VMEM((D, S), _F32),
            pltpu.VMEM((D, S), _F32),
            pltpu.VMEM((4, 2 * HB, H), _BF16),
            pltpu.VMEM((S, D), _BF16),
            pltpu.VMEM((S, S), _BF16),
        ],
        compiler_params=pltpu.CompilerParams(collective_id=0),
    )(q.T, k.T, v.T)
    return out_t.T
```
